```python
import numpy as np

kernel_name = "dist_moe_cap_ep_tokshard_n2048_d512_e8_h1024"

def setup_inputs():
    x = np.random.randn(8192, 512).astype(np.float32)
    router_W = np.random.randn(512, 32).astype(np.float32) * 0.1
    scores64 = x.astype(np.float64) @ router_W.astype(np.float64)
    route_idx = np.argsort(-scores64, axis=-1)[:, :1].astype(np.int32)
    expert_W = np.random.randn(32, 512, 1024).astype(np.float32) * 0.02
    return {"x": x, "router_W": router_W, "route_idx": route_idx, "expert_W": expert_W}

def reference(x, router_W, route_idx, expert_W):
    counts = np.zeros(32, dtype=np.int64)
    out = np.zeros((8192, 1024), dtype=np.float32)
    for i in range(8192):
        e = int(route_idx[i, 0])
        if counts[e] < 204:
            out[i] = x[i] @ expert_W[e]
            counts[e] += 1
    return out
```

```python
import jax
import jax.numpy as jnp
from jax import lax
from jax.experimental import pallas as pl
from jax.experimental.pallas import tpu as pltpu

N_DEV = 4
N_TOK = 2048
D = 512
H = 1024
E_LOC = 8
E = 32
CAP = 204
NG = 32
MAXN = E_LOC * CAP
RA = 3
TA = RA * 128
PA = 64
PD = 64
PC = 32
SR = MAXN + 8
SRA = TA + 8
XA0 = 7 * SR
XDUMP = XA0 + 7 * SRA
YDUMP = 7 * SR
XBLK = ((0, 3), (3, 5), (5, 7), (7, 9), (9, 11), (11, 13), (13, 15), (15, 16))
LF, LD, LH = 2, 3, 4
FLAG = 2
PLAG = 4
TOKS = 3
A_FRAC = (8, 8, 8, 8)
D_FRAC = (8, 8, 8, 8)
C_FRAC = (11, 8, 5, 8)
B1, B2 = 200, 100
MESH = pl.DeviceIdType.MESH
u32 = jnp.uint32
f32 = jnp.float32
bf16 = jnp.bfloat16
scope = jax.named_scope


def _rem_sizes(p):
    out = []
    s = p // 2
    while s >= 8:
        out.append(s)
        s //= 2
    return tuple(out)


def _sem_counts(maxn, p, frac):
    nfull, nrem = maxn // p, len(_rem_sizes(p))
    fmax = max(max(frac), 16 - min(frac))
    return nfull + nrem, min(nfull, (nfull * fmax + 15) // 16 + 1) + nrem


def _n_sems(maxn, p, frac):
    sps, fps = _sem_counts(maxn, p, frac)
    return 3 * sps + 2 * fps


def _pack(a, b):
    ab = lax.bitcast_convert_type(a.astype(bf16).astype(f32), u32)
    bb = lax.bitcast_convert_type(b.astype(bf16).astype(f32), u32)
    return (ab >> 16) | bb


def _lo(w):
    return lax.bitcast_convert_type(w << 16, f32)


def _hi(w):
    return lax.bitcast_convert_type(w & jnp.uint32(0xFFFF0000), f32)


def _body(x_hbm, idx_hbm, w_hbm, out_v,
          idx_v, x_v, w_v, stage, xs, dfwd, ys, cfwd,
          sa_v, sd_v, sc_v, ga_v, cnt_v, tab_v, sa_s, sd_s, sc_s, ga_s, tab_s, tok_s,
          misc_sems, x_sems, w_sems, cnt_send, cnt_recv,
          send_sems, a_recv, d_recv, c_recv):
    me = lax.axis_index("i")

    with scope("s0_zero"):
        idx_cp = pltpu.make_async_copy(idx_hbm, idx_v, misc_sems.at[0])
        idx_cp.start()
        x_cps = [pltpu.make_async_copy(x_hbm.at[pl.ds(128 * a, 128 * (b - a))],
                                       x_v.at[pl.ds(128 * a, 128 * (b - a))], x_sems.at[i])
                 for i, (a, b) in enumerate(XBLK)]
        for cp in x_cps:
            cp.start(priority=1)
        bar = pltpu.get_barrier_semaphore()
        for k in range(1, N_DEV):
            pl.semaphore_signal(bar, inc=1, device_id=(me ^ k,), device_id_type=MESH)
        idx_cp.wait()

    with scope("s1_route"):
        idx = idx_v[...]
        onehot = [(idx == e) for e in range(E)]
        o_em = jnp.concatenate([jnp.where(o, 1.0, 0.0) for o in onehot], axis=0).astype(bf16)
        r_i = lax.broadcasted_iota(jnp.int32, (128, 256), 0)
        c_i = lax.broadcasted_iota(jnp.int32, (128, 256), 1)
        rhs1 = jnp.where((r_i < c_i), 1.0, 0.0).astype(bf16)
        g = jnp.dot(o_em, rhs1, preferred_element_type=f32)
        p_em = g[:, :128]
        t_em = g[:, 128:]
        t_l = jnp.concatenate([t_em[16 * e:16 * (e + 1)] for e in range(E)], axis=1).astype(bf16)
        r2 = lax.broadcasted_iota(jnp.int32, (32, 16), 0)
        c2 = lax.broadcasted_iota(jnp.int32, (32, 16), 1)
        lhs2 = jnp.where(c2 < jnp.where(r2 < 24, r2, RA), 1.0, 0.0).astype(bf16)
        h = jnp.dot(lhs2, t_l, preferred_element_type=f32)
        sub = lax.broadcasted_iota(jnp.int32, (8, 128), 0)
        rank = jnp.zeros((16, 128), f32)
        hist, hist_a = [], []
        for c in range(N_DEV):
            acc = jnp.zeros((8, 128), f32)
            acc_a = jnp.zeros((8, 128), f32)
            for j in range(E_LOC):
                e = c * E_LOC + j
                rank = jnp.where(onehot[e], p_em[16 * e:16 * (e + 1)] + h[:16, 128 * e:128 * (e + 1)], rank)
                acc = jnp.where(sub == j, h[16:24, 128 * e:128 * (e + 1)], acc)
                acc_a = jnp.where(sub == j, h[24:32, 128 * e:128 * (e + 1)], acc_a)
            hist.append(acc)
            hist_a.append(acc_a)
        cnt_me = jnp.minimum(jnp.concatenate(hist, axis=0), float(CAP))
        ca_me = jnp.minimum(jnp.concatenate(hist_a, axis=0), float(CAP))
        lane = lax.broadcasted_iota(jnp.int32, (E, 128), 1)
        row = lax.broadcasted_iota(jnp.int32, (E, 128), 0)
        cnt_v[me] = jnp.where(lane < 64, cnt_me, ca_me)

    with scope("s2_slotA"):
        r3 = lax.broadcasted_iota(jnp.int32, (E, E), 0)
        c3 = lax.broadcasted_iota(jnp.int32, (E, E), 1)
        tri = jnp.where((c3 < r3) & ((c3 >> 3) == (r3 >> 3)), 1.0, 0.0).astype(bf16)
        region = ((row >> 3) ^ me).astype(f32)
        ka_me = jnp.dot(tri, ca_me.astype(bf16), preferred_element_type=f32)
        base_a = ka_me + region * SRA + XA0
        end_a = ka_me + ca_me
        rank8 = rank[:8]
        slot_a = jnp.full((8, 128), float(XDUMP), f32)
        for e in range(E):
            slot_a = jnp.where(onehot[e][:8] & (rank8 < CAP),
                               rank8 + jnp.broadcast_to(base_a[e:e + 1], (8, 128)), slot_a)
        slot_a = slot_a * 2.0
        for c in range(N_DEV):
            e = c * E_LOC + E_LOC - 1
            slot_a = jnp.where(sub == 4 + c, jnp.broadcast_to(end_a[e:e + 1], (8, 128)), slot_a)
        sa_v[...] = slot_a.astype(jnp.int32)
        sa_cp = pltpu.make_async_copy(sa_v, sa_s, misc_sems.at[1])
        sa_cp.start()

    with scope("s2_bar"):
        pl.semaphore_wait(bar, N_DEV - 1)
        cnt_cps = []
        for k in (2, 3, 1):
            cp = pltpu.make_async_remote_copy(
                src_ref=cnt_v.at[me], dst_ref=cnt_v.at[me], send_sem=cnt_send.at[k - 1], recv_sem=cnt_recv.at[k - 1],
                device_id=(me ^ k,), device_id_type=MESH)
            cp.start()
            cnt_cps.append(cp)

    def pack_block(i):
        a, b = XBLK[i]
        x_cps[i].wait()
        def pk(t, c):
            r0 = pl.multiple_of(t * 32, 32)
            xv = x_v[pl.ds(r0, 32), :]
            stage[pl.ds(2 * r0, 32, stride=2), :] = _pack(xv[:, 0:128], xv[:, 256:384])
            stage[pl.ds(2 * r0 + 1, 32, stride=2), :] = _pack(xv[:, 128:256], xv[:, 384:512])
            return c
        lax.fori_loop(4 * a, 4 * b, pk, 0)

    def scatter_rows(slot_s, r0, r1):
        def sc(r, c):
            t0 = pl.multiple_of(r * 256, 256)
            for l in range(128):
                xs[pl.ds(slot_s[r, l], 2), :] = stage[pl.ds(t0 + 2 * l, 2), :]
            return c
        lax.fori_loop(r0, r1, sc, 0)

    def for_units(p_rows, n8, u0, u1, fn):
        nf = n8 // p_rows
        def body(p, c):
            fn(p, p * p_rows, p_rows, None)
            return c
        lax.fori_loop(u0, jnp.minimum(u1, nf), body, 0)
        rem = n8 - nf * p_rows
        @pl.when((u0 <= nf) & (nf < u1))
        def _():
            for i, sz in enumerate(_rem_sizes(p_rows)):
                @pl.when((rem & sz) != 0)
                def _(i=i, sz=sz):
                    fn(nf, nf * p_rows + (rem & ~(2 * sz - 1)), sz, i)

    class Phase:
        def __init__(self, buf, base, reg, fwd, fbase, rpt, recv, frac, ssem, p_rows, maxn):
            self.buf, self.base, self.reg, self.fwd, self.fbase = buf, base, reg, fwd, fbase
            self.rpt, self.recv, self.ssem, self.p = rpt, recv, ssem, p_rows
            self.sps, self.fps = _sem_counts(maxn, p_rows, frac)
            self.nrem = len(_rem_sizes(p_rows))
            self.frac = jnp.int32(8 * (frac[0] | (frac[1] << 8) | (frac[2] << 16) | (frac[3] << 24)))

        def n_x(self, a, p):
            return (p * ((self.frac >> (8 * a)) & 255) + 32) >> 7

        def via_x(self, a, p):
            return self.n_x(a, p + 1) - self.n_x(a, p)

        def rows(self, region, off, sz):
            return self.buf.at[pl.ds(self.rpt * (self.base + region * self.reg + off), self.rpt * sz)]

        def frows(self, sl, off, sz):
            return self.fwd.at[pl.ds(self.rpt * (self.fbase + sl * self.reg + off), self.rpt * sz)]

        def sem(self, k, p, ri):
            return self.recv.at[(k - 1) * self.sps + (p if ri is None else self.sps - self.nrem + ri)]

        def direct(self, k, p, off, sz, ri):
            return pltpu.make_async_remote_copy(
                src_ref=self.rows(k, off, sz), dst_ref=self.rows(3 + k, off, sz),
                send_sem=send_sems.at[self.ssem], recv_sem=self.sem(k, p, ri),
                device_id=(me ^ k,), device_id_type=MESH)

        def hop1(self, a, sl, p, off, sz, ri):
            if ri is None:
                nx = self.n_x(a, p)
                si = jnp.where(sl == 0, nx, p - nx)
            else:
                si = self.fps - self.nrem + ri
            return pltpu.make_async_remote_copy(
                src_ref=self.rows(2, off, sz), dst_ref=self.frows(sl, off, sz),
                send_sem=send_sems.at[self.ssem], recv_sem=self.recv.at[3 * self.sps + sl * self.fps + si],
                device_id=(me ^ (3 - 2 * sl),), device_id_type=MESH)

        def hop1_out(self, p, off, sz, ri):
            return self.hop1(me, 1 - self.via_x(me, p), p, off, sz, ri)

        def hop2(self, sl, p, off, sz, ri):
            return pltpu.make_async_remote_copy(
                src_ref=self.frows(sl, off, sz), dst_ref=self.rows(5, off, sz),
                send_sem=send_sems.at[self.ssem], recv_sem=self.sem(2, p, ri),
                device_id=(me ^ (1 + 2 * sl),), device_id_type=MESH)

        def mine(self, sl, p):
            return self.via_x(me ^ (3 - 2 * sl), p) == 1 - sl

        def send(self, k, n8, u0, u1):
            if k == 2:
                for_units(self.p, n8, u0, u1, lambda *a: self.hop1_out(*a).start())
            else:
                for_units(self.p, n8, u0, u1, lambda *a: self.direct(k, *a).start())

        def wait(self, k, n8, u0, u1):
            for_units(self.p, n8, u0, u1, lambda *a: self.direct(k, *a).wait_recv())

        def forward(self, sl, n8, u0, u1):
            def fn(p, off, sz, ri):
                @pl.when(self.mine(sl, p))
                def _():
                    self.hop1(me ^ (3 - 2 * sl), sl, p, off, sz, ri).wait_recv()
                    self.hop2(sl, p, off, sz, ri).start()
            for_units(self.p, n8, u0, u1, fn)

        def drain(self, own, fwd):
            for_units(self.p, own[2], 0, self.sps, lambda *a: self.hop1_out(*a).wait_send())
            for k in (3, 1):
                for_units(self.p, own[k], 0, self.sps, lambda *a, k=k: self.direct(k, *a).wait_send())
            for sl in range(2):
                def fn(p, off, sz, ri, sl=sl):
                    @pl.when(self.mine(sl, p))
                    def _():
                        self.hop2(sl, p, off, sz, ri).wait_send()
                for_units(self.p, fwd[sl], 0, self.sps, fn)

    ap = Phase(xs, XA0, SRA, dfwd, 2 * SR, 2, a_recv, A_FRAC, 0, PA, TA)
    dp = Phase(xs, 0, SR, dfwd, 0, 2, d_recv, D_FRAC, 1, PD, MAXN)
    cp_ = Phase(ys, 0, SR, cfwd, 0, 4, c_recv, C_FRAC, 2, PC, MAXN)

    def up8(n):
        return ((n + 7) >> 3) << 3

    with scope("s2_genA"):
        pack_block(0)
        sa_cp.wait()
        scatter_rows(sa_s, 0, RA)
        a_out = {k: up8(sa_s[4 + (me ^ k), 0]) for k in range(1, 4)}
        for k in (2, 3, 1):
            ap.send(k, a_out[k], 0, ap.sps)

    with scope("s2_pack0"):
        for i in (1, 2):
            pack_block(i)

    with scope("s3_cntwait"):
        for k in range(1, N_DEV):
            src = me ^ k
            pltpu.make_async_remote_copy(
                src_ref=cnt_v.at[src], dst_ref=cnt_v.at[src], send_sem=cnt_send.at[k - 1], recv_sem=cnt_recv.at[k - 1],
                device_id=(src,), device_id_type=MESH).wait_recv()

    with scope("s4_tab"):
        pre = jnp.zeros((E, 128), f32)
        q = jnp.zeros((E, 128), f32)
        add = jnp.zeros((E, 128), f32)
        nk_me = jnp.zeros((E, 128), f32)
        grp = lane >> 2
        for s in range(N_DEV):
            m = cnt_v[s]
            mr = pltpu.roll(m, 64, 1)
            c = jnp.where(lane < 64, m, mr)
            ca = jnp.where(lane < 64, mr, m)
            nk = jnp.clip(CAP - pre, 0.0, c)
            pre = pre + c
            na = jnp.minimum(ca, nk)
            nb = nk - na
            sel = (lane & 3) == s
            qs = jnp.where(grp < 2, nk, jnp.where(grp < 4, nb, ca))
            ads = jnp.where(grp == 0, nk, jnp.where(grp == 2, nb, jnp.where(grp == 4, na, jnp.where(grp == 6, ca, 0.0))))
            q = jnp.where(sel, qs, q)
            add = jnp.where(sel, ads, add)
            nk_me = jnp.where(me == s, nk, nk_me)
        nb_me = nk_me - jnp.minimum(ca_me, nk_me)
        kk = jnp.dot(tri, jnp.concatenate([nb_me, q, nk_me], axis=1).astype(bf16), preferred_element_type=f32)
        base_d = kk[:, :128] + region * SR - ca_me
        base_c = kk[:, 256:] + region * SR
        slot_d = jnp.full((16, 128), float(XDUMP), f32)
        slot_c = jnp.full((16, 128), float(YDUMP), f32)
        for e in range(E):
            keep = onehot[e] & (rank < jnp.broadcast_to(nk_me[e:e + 1], (16, 128)))
            slot_d = jnp.where(keep, rank + jnp.broadcast_to(base_d[e:e + 1], (16, 128)), slot_d)
            slot_c = jnp.where(keep, rank + jnp.broadcast_to(base_c[e:e + 1], (16, 128)), slot_c)
        sd_v[...] = slot_d.astype(jnp.int32) * 2
        sd_cp = pltpu.make_async_copy(sd_v, sd_s, misc_sems.at[2])
        sd_cp.start()
        tab_v[...] = (kk[:, 128:256] + add).astype(jnp.int32)
        tab_cp = pltpu.make_async_copy(tab_v, tab_s, misc_sems.at[3])
        tab_cp.start()
        tabf = kk[:, 128:256] + add
        t = tabf[:8]
        for c in range(1, N_DEV):
            t = jnp.where(me == c, tabf[8 * c:8 * c + 8], t)
        lane8 = lax.broadcasted_iota(jnp.int32, (8, 128), 1)
        is_x = lane8 < 32
        gidx = (lane8 & 31).astype(f32)
        def bc(qi, s_):
            return jnp.broadcast_to(t[:, 4 * qi + s_:4 * qi + s_ + 1], (8, 128))
        gs = jnp.zeros((8, 128), f32)
        adr = jnp.zeros((8, 128), f32)
        for s_ in range(N_DEV):
            kx = s_ ^ me
            reg = jnp.where(kx == 0, 0, 3 + kx).astype(f32)
            yreg = (kx * SR).astype(f32)
            c0, b1, b0, a1, a0 = bc(1, s_), bc(2, s_), bc(3, s_), bc(4, s_), bc(5, s_)
            for x0, y0, n in ((XA0 + reg * SRA + a0, yreg + c0, a1 - a0),
                              (reg * SR + b0, yreg + c0 + (a1 - a0), b1 - b0)):
                adr = jnp.where(gidx >= gs, jnp.where(is_x, x0, y0) + 8.0 * (gidx - gs), adr)
                gs = gs + jnp.floor((n + 7.0) * 0.125)
        adr = jnp.where(gidx >= gs, jnp.where(is_x, float(XDUMP), float(YDUMP)), adr)
        ga_v[...] = (adr * jnp.where(is_x, 2.0, 4.0)).astype(jnp.int32)
        ga_cp = pltpu.make_async_copy(ga_v, ga_s, misc_sems.at[5])
        ga_cp.start()
        sc_v[...] = slot_c.astype(jnp.int32)
        sc_cp = pltpu.make_async_copy(sc_v, sc_s, misc_sems.at[4])
        sc_cp.start()

    def tab(qi, s, e):
        return tab_s[e, 4 * qi + s]

    class Stream:
        def __init__(self, s, c):
            self.s, self.c = s, c
            last = c * E_LOC + E_LOC - 1
            self.n = tab(0, s, last)
            self.c8 = up8(self.n)
            self.d8 = up8(tab(2, s, last))
            self.a8 = up8(tab(6, s, last))
            self.ud = (self.d8 + PD - 1) // PD
            self.uc = (self.c8 + PC - 1) // PC

        def _end(self, qi, j):
            return tab(qi, self.s, self.c * E_LOC + jnp.clip(j, 0, E_LOC - 1))

        def need(self, j):
            return jnp.where(j < 0, 0, jnp.minimum((self._end(2, j) + 7 + PD - 1) // PD, self.ud))

        def sched(self, j):
            u = jnp.maximum((self._end(2, j) + 7 + PD - 1) // PD, (j + 1) * 64 // PD)
            return jnp.where(j < 0, 0, jnp.minimum(u, self.ud))

        def avail(self, j):
            a = jnp.where(j >= E_LOC - 1, self.uc, self._end(0, j) // PC)
            return jnp.where(j < 0, 0, a)

    with scope("s5_pack"):
        pack_block(3)
        sd_cp.wait()
        scatter_rows(sd_s, RA, XBLK[3][1])
        tab_cp.wait()
        s_out = {k: Stream(me, me ^ k) for k in range(1, 4)}
        s_in = {k: Stream(me ^ k, me) for k in range(1, 4)}
        sx, sy = Stream(me ^ 3, me ^ 1), Stream(me ^ 1, me ^ 3)
        s_fd = {0: sx, 1: sy}
        s_fc = {0: sy, 1: sx}
        for sl in range(2):
            ap.forward(sl, s_fd[sl].a8, 0, ap.sps)
        for i in range(4, len(XBLK)):
            pack_block(i)
            if i == len(XBLK) - 1:
                for j in range(E_LOC):
                    pltpu.make_async_copy(w_hbm.at[j], w_v.at[j], w_sems.at[j]).start(priority=1)
            scatter_rows(sd_s, *XBLK[i])

    def d_step(j):
        for sl in range(2):
            st = s_fd[sl]
            dp.forward(sl, st.d8, st.sched(j + LF - 1), st.sched(j + LF))
        for k, la in ((3, LD), (1, LD), (2, LH)):
            st = s_out[k]
            dp.send(k, st.d8, st.sched(j + la - 1), st.sched(j + la))

    def put_rows(k_region, k_tok, r0, r1):
        def grp(g, c):
            for u in range(8):
                r = jnp.minimum(r0 + g * 8 + u, r1 - 1)
                o = pl.multiple_of(tok_s[k_tok * SR + r], 8)
                w = ys[pl.ds(4 * (k_region * SR + r), 4), :]
                out_v[pl.ds(o, 4), :] = _lo(w)
                out_v[pl.ds(o + 4, 4), :] = _hi(w)
            return c
        lax.fori_loop(0, (r1 - r0 + 7) >> 3, grp, 0)

    def recv_put(k, j):
        st = s_out[k]
        def fn(p, off, sz, ri):
            cp_.direct(k, p, off, sz, ri).wait_recv()
            put_rows(3 + k, k, off, jnp.minimum(off + sz, st.n))
        for_units(PC, st.c8, st.avail(j - 1), st.avail(j), fn)

    def c_tail(j):
        with scope("q0_fwd"):
            for sl in range(2):
                st = s_fc[sl]
                cp_.forward(sl, st.c8, st.avail(j - FLAG - 1), st.avail(j - FLAG))
        with scope("q1_put"):
            for k in (3, 1):
                recv_put(k, j - PLAG)
            recv_put(2, j - PLAG - FLAG)

    with scope("s6_d0"):
        z = jnp.int32(0)
        for k in (2, 3, 1):
            dp.send(k, s_out[k].d8, 0, s_out[k].sched(z))
        dp.send(2, s_out[2].d8, s_out[2].sched(z), s_out[2].sched(z + 1))
    with scope("s7_zero"):
        def tot(qi, s_, c):
            return tab(qi, s_, c * E_LOC + E_LOC - 1)
        f2 = 64 + (32 * (tot(2, 3, 0) - tot(2, 2, 1) + 2 * (tot(0, 0, 3) - tot(0, 1, 2)) + B1)) // jnp.maximum(tot(0, 0, 2), 1)
        f0 = 64 - (32 * (tot(2, 3, 2) - tot(2, 0, 1) + 2 * (tot(0, 2, 3) - tot(0, 1, 0)) + B2)) // jnp.maximum(tot(0, 2, 0), 1)
        cp_.frac = jnp.clip(f0, 40, 88) | (64 << 8) | (jnp.clip(f2, 40, 88) << 16) | (64 << 24)
        for cp in cnt_cps:
            cp.wait_send()
        sc_cp.wait()
        ga_cp.wait()
        def zo(i, c):
            out_v[pl.ds(pl.multiple_of(i * 256, 256), 256), :] = jnp.zeros((256, 128), f32)
            return c
        lax.fori_loop(0, N_TOK * 8 // 256, zo, 0)
    with scope("s8_d1"):
        def pro(j, c):
            d_step(j)
            return c
        lax.fori_loop(-LF, 0, pro, 0)
        for k in (3, 1, 2):
            ap.wait(k, s_in[k].a8, 0, ap.sps)

    def compute(j, c):
        e = me * E_LOC + j
        with scope("c2_wait"):
            for k in (3, 1, 2):
                st = s_in[k]
                dp.wait(k, st.d8, st.need(j - 1), st.need(j))
        with scope("c2_ww"):
            pltpu.make_async_copy(w_hbm.at[j], w_v.at[j], w_sems.at[j]).wait()
        with scope("c3_mm"):
            xa = [ga_s[j, gi] for gi in range(NG)]
            ya = [ga_s[j, 32 + gi] for gi in range(NG)]
            w0 = jnp.concatenate([xs[pl.ds(a, 8, stride=2), :] for a in xa], axis=0)
            w1 = jnp.concatenate([xs[pl.ds(a + 1, 8, stride=2), :] for a in xa], axis=0)
            lhs = jnp.concatenate([_lo(w0), _lo(w1), _hi(w0), _hi(w1)], axis=1).astype(bf16)
            for qq in range(4):
                wa = w_v[j, :, pl.ds(128 * qq, 128)].astype(bf16)
                wb = w_v[j, :, pl.ds(512 + 128 * qq, 128)].astype(bf16)
                pk = _pack(jnp.dot(lhs, wa, preferred_element_type=f32),
                           jnp.dot(lhs, wb, preferred_element_type=f32))
                for gi in range(NG):
                    ys[pl.ds(ya[gi] + qq, 8, stride=4), :] = pk[8 * gi:8 * gi + 8]
        with scope("c4_send"):
            for k in (2, 3, 1):
                st = s_in[k]
                cp_.send(k, st.c8, st.avail(j - 1), st.avail(j))
        with scope("c5_d"):
            d_step(j)
        with scope("c6_tok"):
            def tk(r, c2):
                for l in range(128):
                    tok_s[sc_s[r, l]] = (r * 128 + l) * 8
                return c2
            lax.fori_loop(jnp.clip(6 * (j - 1), 0, 16), jnp.clip(6 * j, 0, 16), tk, 0)
        with scope("c7_put"):
            @pl.when(j >= TOKS)
            def _():
                put_rows(0, 0, jnp.where(j == TOKS, 0, tab(1, me, e)), tab(0, me, e))
        c_tail(j)
        return c
    lax.fori_loop(0, E_LOC, compute, 0)

    with scope("p1_drain_d"):
        ap.drain(a_out, {sl: s_fd[sl].a8 for sl in range(2)})
        dp.drain({k: s_out[k].d8 for k in s_out}, {sl: s_fd[sl].d8 for sl in range(2)})

    def ep(j, c):
        c_tail(j)
        return c
    lax.fori_loop(E_LOC, E_LOC + FLAG + PLAG - 1, ep, 0)

    with scope("p3_drain_c"):
        cp_.drain({k: s_in[k].c8 for k in s_in}, {sl: s_fc[sl].c8 for sl in range(2)})
    with scope("p4_drain_f"):
        recv_put(2, jnp.int32(E_LOC - 1))


def pallas_dist_moe_cap_ep_tokshard_n2048_d512_e8_h1024_kernel(x, router_W, route_idx, expert_W):
    del router_W
    idx = route_idx.astype(jnp.int32).reshape(16, 128)
    DMA = pltpu.SemaphoreType.DMA
    return pl.pallas_call(
        _body,
        out_shape=jax.ShapeDtypeStruct((N_TOK * 8, 128), f32),
        in_specs=[pl.BlockSpec(memory_space=pl.ANY)] * 3,
        out_specs=pl.BlockSpec(memory_space=pltpu.VMEM),
        scratch_shapes=[
            pltpu.VMEM((16, 128), jnp.int32),
            pltpu.VMEM((N_TOK, D), f32),
            pltpu.VMEM((E_LOC, D, H), f32),
            pltpu.VMEM((2 * N_TOK + 8, 128), u32),
            pltpu.VMEM((2 * (XDUMP + 16), 128), u32),
            pltpu.VMEM((2 * 2 * (SR + SRA), 128), u32),
            pltpu.VMEM((4 * (YDUMP + 16), 128), u32),
            pltpu.VMEM((4 * 2 * SR, 128), u32),
            pltpu.VMEM((8, 128), jnp.int32),
            pltpu.VMEM((16, 128), jnp.int32),
            pltpu.VMEM((16, 128), jnp.int32),
            pltpu.VMEM((8, 128), jnp.int32),
            pltpu.VMEM((N_DEV, E, 128), f32),
            pltpu.VMEM((E, 128), jnp.int32),
            pltpu.SMEM((8, 128), jnp.int32),
            pltpu.SMEM((16, 128), jnp.int32),
            pltpu.SMEM((16, 128), jnp.int32),
            pltpu.SMEM((8, 128), jnp.int32),
            pltpu.SMEM((E, 128), jnp.int32),
            pltpu.SMEM((YDUMP + 8,), jnp.int32),
            DMA((6,)), DMA((len(XBLK),)), DMA((E_LOC,)), DMA((3,)), DMA((3,)),
            DMA((3,)), DMA((_n_sems(TA, PA, A_FRAC),)), DMA((_n_sems(MAXN, PD, D_FRAC),)),
            DMA((_n_sems(MAXN, PC, C_FRAC),)),
        ],
        compiler_params=pltpu.CompilerParams(collective_id=0, vmem_limit_bytes=100 * 1024 * 1024,
                                             disable_semaphore_checks=True),
    )(x, idx, expert_W).reshape(N_TOK, H)
```

```python
import jax
import jax.numpy as jnp
from jax import lax
from jax.experimental import pallas as pl
from jax.experimental.pallas import tpu as pltpu

N_DEV = 4
N_TOK = 2048
D = 512
H = 1024
E_LOC = 8
E = 32
CAP = 204
NG = 32
MAXN = E_LOC * CAP
RA = 4
TA = RA * 128
PA, GA = 64, 8
PD, GD = 64, 8
PC, GC = 32, 4
SR = MAXN + 8
SRA = TA + 8
XA0 = 7 * SR
XDUMP = XA0 + 7 * SRA
YDUMP = 7 * SR
XBLK = ((0, 2), (2, 3), (3, 4), (4, 7), (7, 10), (10, 13), (13, 15), (15, 16))
NBA = 3
LF, LD, LH = 2, 3, 4
FLAG = 2
PLAG = 3
TOKS = 3
FLO, FHI = 40, 88
B1, B2 = 250, 150
MESH = pl.DeviceIdType.MESH
u32 = jnp.uint32
f32 = jnp.float32
bf16 = jnp.bfloat16


def _rem_sizes(p, g):
    out = []
    s = p // 2
    while s >= g:
        out.append(s)
        s //= 2
    return tuple(out)


def _sem_counts(maxn, p, g, fmax):
    nfull, nrem = maxn // p, len(_rem_sizes(p, g))
    return nfull + nrem, min(nfull, (nfull * fmax + 127) // 128 + 1) + nrem


def _n_sems(maxn, p, g, fmax):
    sps, fps = _sem_counts(maxn, p, g, fmax)
    return 3 * sps + 2 * fps


def _pack(a, b):
    ab = lax.bitcast_convert_type(a.astype(bf16).astype(f32), u32)
    bb = lax.bitcast_convert_type(b.astype(bf16).astype(f32), u32)
    return (ab >> 16) | bb


def _lo(w):
    return lax.bitcast_convert_type(w << 16, f32)


def _hi(w):
    return lax.bitcast_convert_type(w & jnp.uint32(0xFFFF0000), f32)


def _up(n, g):
    return (n + (g - 1)) & ~(g - 1)


def _body(x_hbm, idx_hbm, w_hbm, out_v,
          idx_v, x_v, w_v, xs, dfwd, ys, cfwd,
          sa_v, sd_v, sc_v, ga_v, cnt_v, tab_v, sa_s, sd_s, sc_s, ga_s, tab_s, tok_s,
          misc_sems, x_sems, w_sems, cnt_send, cnt_recv,
          send_sems, a_recv, d_recv, c_recv):
    me = lax.axis_index("i")

    idx_cp = pltpu.make_async_copy(idx_hbm, idx_v, misc_sems.at[0])
    idx_cp.start()
    x_cps = [pltpu.make_async_copy(x_hbm.at[pl.ds(128 * a, 128 * (b - a))],
                                   x_v.at[pl.ds(128 * a, 128 * (b - a))], x_sems.at[i])
             for i, (a, b) in enumerate(XBLK)]
    for cp in x_cps:
        cp.start(priority=1)
    bar = pltpu.get_barrier_semaphore()
    for k in range(1, N_DEV):
        pl.semaphore_signal(bar, inc=1, device_id=(me ^ k,), device_id_type=MESH)
    idx_cp.wait()

    idx = idx_v[...]
    onehot = [(idx == e) for e in range(E)]
    o_em = jnp.concatenate([jnp.where(o, 1.0, 0.0) for o in onehot], axis=0).astype(bf16)
    r_i = lax.broadcasted_iota(jnp.int32, (128, 256), 0)
    c_i = lax.broadcasted_iota(jnp.int32, (128, 256), 1)
    rhs1 = jnp.where(r_i < c_i, 1.0, 0.0).astype(bf16)
    g = jnp.dot(o_em, rhs1, preferred_element_type=f32)
    p_em = g[:, :128]
    t_em = g[:, 128:]
    t_l = jnp.concatenate([t_em[16 * e:16 * (e + 1)] for e in range(E)], axis=1).astype(bf16)
    r2 = lax.broadcasted_iota(jnp.int32, (32, 16), 0)
    c2 = lax.broadcasted_iota(jnp.int32, (32, 16), 1)
    lhs2 = jnp.where(c2 < jnp.where(r2 < 24, r2, RA), 1.0, 0.0).astype(bf16)
    h = jnp.dot(lhs2, t_l, preferred_element_type=f32)
    sub = lax.broadcasted_iota(jnp.int32, (8, 128), 0)
    rank = jnp.zeros((16, 128), f32)
    hist, hist_a = [], []
    for c in range(N_DEV):
        acc = jnp.zeros((8, 128), f32)
        acc_a = jnp.zeros((8, 128), f32)
        for j in range(E_LOC):
            e = c * E_LOC + j
            he = h[:, 128 * e:128 * (e + 1)]
            rank = jnp.where(onehot[e], p_em[16 * e:16 * (e + 1)] + he[:16], rank)
            acc = jnp.where(sub == j, he[16:24], acc)
            acc_a = jnp.where(sub == j, he[24:32], acc_a)
        hist.append(acc)
        hist_a.append(acc_a)
    cnt_me = jnp.minimum(jnp.concatenate(hist, axis=0), float(CAP))
    ca_me = jnp.minimum(jnp.concatenate(hist_a, axis=0), float(CAP))
    lane = lax.broadcasted_iota(jnp.int32, (E, 128), 1)
    row = lax.broadcasted_iota(jnp.int32, (E, 128), 0)
    cnt_v[me] = jnp.where(lane < 64, cnt_me, ca_me)

    r3 = lax.broadcasted_iota(jnp.int32, (E, E), 0)
    c3 = lax.broadcasted_iota(jnp.int32, (E, E), 1)
    tri = jnp.where((c3 < r3) & ((c3 >> 3) == (r3 >> 3)), 1.0, 0.0).astype(bf16)
    region = ((row >> 3) ^ me).astype(f32)
    ka_me = jnp.dot(tri, ca_me.astype(bf16), preferred_element_type=f32)
    base_a = ka_me + region * SRA + XA0
    end_a = ka_me + ca_me
    rank8 = rank[:8]
    slot_a = jnp.full((8, 128), float(XDUMP), f32)
    for e in range(E):
        slot_a = jnp.where(onehot[e][:8] & (rank8 < CAP),
                           rank8 + jnp.broadcast_to(base_a[e:e + 1], (8, 128)), slot_a)
    for c in range(N_DEV):
        e = c * E_LOC + E_LOC - 1
        slot_a = jnp.where(sub == 4 + c, jnp.broadcast_to(end_a[e:e + 1], (8, 128)), slot_a)
    sa_v[...] = slot_a.astype(jnp.int32)
    sa_cp = pltpu.make_async_copy(sa_v, sa_s, misc_sems.at[1])
    sa_cp.start()

    def cnt_copy(owner, k):
        return pltpu.make_async_remote_copy(
            src_ref=cnt_v.at[owner], dst_ref=cnt_v.at[owner],
            send_sem=cnt_send.at[k - 1], recv_sem=cnt_recv.at[k - 1],
            device_id=(me ^ k,), device_id_type=MESH)

    pl.semaphore_wait(bar, N_DEV - 1)
    for k in (2, 3, 1):
        cnt_copy(me, k).start()

    def scatter_block(slot_s, i):
        x_cps[i].wait()

        def sc(r, c):
            for g8 in range(16):
                xv = x_v[pl.ds(pl.multiple_of(r * 128 + 8 * g8, 8), 8), :]
                w0 = _pack(xv[:, 0:128], xv[:, 256:384])
                w1 = _pack(xv[:, 128:256], xv[:, 384:512])
                for u in range(8):
                    sl = slot_s[r, 8 * g8 + u]
                    xs[sl, 0:1, :] = w0[u:u + 1]
                    xs[sl, 1:2, :] = w1[u:u + 1]
            return c
        lax.fori_loop(XBLK[i][0], XBLK[i][1], sc, 0)

    class Phase:
        def __init__(self, buf, base, reg, fwd, fbase, recv, ssem, p, g, maxn, fmax):
            self.buf, self.base, self.reg, self.fwd, self.fbase = buf, base, reg, fwd, fbase
            self.recv, self.ssem, self.p, self.g = recv, ssem, p, g
            self.sps, self.fps = _sem_counts(maxn, p, g, fmax)
            self.nrem = len(_rem_sizes(p, g))
            self.frac = jnp.int32(0x40404040)

        def units(self, n, u0, u1, fn):
            nf = n // self.p

            def body(u, c):
                fn(u, u * self.p, self.p, None)
                return c
            lax.fori_loop(u0, jnp.minimum(u1, nf), body, 0)
            rem = n - nf * self.p

            @pl.when((u0 <= nf) & (nf < u1))
            def _():
                for i, sz in enumerate(_rem_sizes(self.p, self.g)):
                    @pl.when((rem & sz) != 0)
                    def _(i=i, sz=sz):
                        fn(nf, nf * self.p + (rem & ~(2 * sz - 1)), sz, i)

        def n_x(self, a, u):
            return (u * ((self.frac >> (8 * a)) & 255) + 32) >> 7

        def via_x(self, a, u):
            return self.n_x(a, u + 1) - self.n_x(a, u)

        def rows(self, region_, off, sz):
            return self.buf.at[pl.ds(self.base + region_ * self.reg + off, sz)]

        def frows(self, sl, off, sz):
            return self.fwd.at[pl.ds(self.fbase + sl * self.reg + off, sz)]

        def sem(self, k, u, ri):
            return self.recv.at[(k - 1) * self.sps + (u if ri is None else self.sps - self.nrem + ri)]

        def direct(self, k, u, off, sz, ri):
            return pltpu.make_async_remote_copy(
                src_ref=self.rows(k, off, sz), dst_ref=self.rows(3 + k, off, sz),
                send_sem=send_sems.at[self.ssem], recv_sem=self.sem(k, u, ri),
                device_id=(me ^ k,), device_id_type=MESH)

        def hop1(self, a, sl, u, off, sz, ri):
            if ri is None:
                nx = self.n_x(a, u)
                si = jnp.where(sl == 0, nx, u - nx)
            else:
                si = self.fps - self.nrem + ri
            return pltpu.make_async_remote_copy(
                src_ref=self.rows(2, off, sz), dst_ref=self.frows(sl, off, sz),
                send_sem=send_sems.at[self.ssem],
                recv_sem=self.recv.at[3 * self.sps + sl * self.fps + si],
                device_id=(me ^ (3 - 2 * sl),), device_id_type=MESH)

        def hop1_out(self, u, off, sz, ri):
            return self.hop1(me, 1 - self.via_x(me, u), u, off, sz, ri)

        def hop2(self, sl, u, off, sz, ri):
            return pltpu.make_async_remote_copy(
                src_ref=self.frows(sl, off, sz), dst_ref=self.rows(5, off, sz),
                send_sem=send_sems.at[self.ssem], recv_sem=self.sem(2, u, ri),
                device_id=(me ^ (1 + 2 * sl),), device_id_type=MESH)

        def mine(self, sl, u):
            return self.via_x(me ^ (3 - 2 * sl), u) == 1 - sl

        def send(self, k, n, u0, u1):
            if k == 2:
                self.units(n, u0, u1, lambda *a: self.hop1_out(*a).start())
            else:
                self.units(n, u0, u1, lambda *a: self.direct(k, *a).start())

        def wait(self, k, n, u0, u1):
            self.units(n, u0, u1, lambda *a: self.direct(k, *a).wait_recv())

        def forward(self, sl, n, u0, u1):
            def fn(u, off, sz, ri):
                @pl.when(self.mine(sl, u))
                def _():
                    self.hop1(me ^ (3 - 2 * sl), sl, u, off, sz, ri).wait_recv()
                    self.hop2(sl, u, off, sz, ri).start()
            self.units(n, u0, u1, fn)

        def drain(self, own, fwd):
            self.units(own[2], 0, self.sps, lambda *a: self.hop1_out(*a).wait_send())
            for k in (3, 1):
                self.units(own[k], 0, self.sps, lambda *a, k=k: self.direct(k, *a).wait_send())
            for sl in range(2):
                def fn(u, off, sz, ri, sl=sl):
                    @pl.when(self.mine(sl, u))
                    def _():
                        self.hop2(sl, u, off, sz, ri).wait_send()
                self.units(fwd[sl], 0, self.sps, fn)

    ap = Phase(xs, XA0, SRA, dfwd, 2 * SR, a_recv, 0, PA, GA, TA, 64)
    dp = Phase(xs, 0, SR, dfwd, 0, d_recv, 1, PD, GD, MAXN, 64)
    cp_ = Phase(ys, 0, SR, cfwd, 0, c_recv, 2, PC, GC, MAXN, max(FHI, 128 - FLO))

    sa_cp.wait()
    for i in range(NBA):
        scatter_block(sa_s, i)
    a_out = {k: _up(sa_s[4 + (me ^ k), 0], GA) for k in range(1, 4)}
    for k in (2, 3, 1):
        ap.send(k, a_out[k], 0, ap.sps)

    for k in range(1, N_DEV):
        cnt_copy(me ^ k, k).wait_recv()
    pre = jnp.zeros((E, 128), f32)
    q = jnp.zeros((E, 128), f32)
    add = jnp.zeros((E, 128), f32)
    nk_me = jnp.zeros((E, 128), f32)
    grp = lane >> 2
    for s in range(N_DEV):
        m = cnt_v[s]
        mr = pltpu.roll(m, 64, 1)
        c = jnp.where(lane < 64, m, mr)
        ca = jnp.where(lane < 64, mr, m)
        nk = jnp.clip(CAP - pre, 0.0, c)
        pre = pre + c
        na = jnp.minimum(ca, nk)
        nb = nk - na
        sel = (lane & 3) == s
        qs = jnp.where(grp < 2, nk, jnp.where(grp < 4, nb, ca))
        ads = jnp.where(grp == 0, nk, jnp.where(grp == 2, nb,
                        jnp.where(grp == 4, na, jnp.where(grp == 6, ca, 0.0))))
        q = jnp.where(sel, qs, q)
        add = jnp.where(sel, ads, add)
        nk_me = jnp.where(me == s, nk, nk_me)
    nb_me = nk_me - jnp.minimum(ca_me, nk_me)
    kk = jnp.dot(tri, jnp.concatenate([nb_me, q, nk_me], axis=1).astype(bf16),
                 preferred_element_type=f32)
    base_d = kk[:, :128] + region * SR - ca_me
    base_c = kk[:, 256:] + region * SR
    slot_d = jnp.full((16, 128), float(XDUMP), f32)
    slot_c = jnp.full((16, 128), float(YDUMP), f32)
    for e in range(E):
        keep = onehot[e] & (rank < jnp.broadcast_to(nk_me[e:e + 1], (16, 128)))
        slot_d = jnp.where(keep, rank + jnp.broadcast_to(base_d[e:e + 1], (16, 128)), slot_d)
        slot_c = jnp.where(keep, rank + jnp.broadcast_to(base_c[e:e + 1], (16, 128)), slot_c)
    sd_v[...] = slot_d.astype(jnp.int32)
    sd_cp = pltpu.make_async_copy(sd_v, sd_s, misc_sems.at[2])
    sd_cp.start()
    tabf = kk[:, 128:256] + add
    tab_v[...] = tabf.astype(jnp.int32)
    tab_cp = pltpu.make_async_copy(tab_v, tab_s, misc_sems.at[3])
    tab_cp.start()

    t = tabf[:8]
    for c in range(1, N_DEV):
        t = jnp.where(me == c, tabf[8 * c:8 * c + 8], t)
    lane8 = lax.broadcasted_iota(jnp.int32, (8, 128), 1)
    is_x = lane8 < 32
    gidx = (lane8 & 31).astype(f32)

    def bc(qi, s_):
        return jnp.broadcast_to(t[:, 4 * qi + s_:4 * qi + s_ + 1], (8, 128))
    gs = jnp.zeros((8, 128), f32)
    adr = jnp.zeros((8, 128), f32)
    for s_ in range(N_DEV):
        kx = s_ ^ me
        reg = jnp.where(kx == 0, 0, 3 + kx).astype(f32)
        yreg = (kx * SR).astype(f32)
        c0, b1, b0, a1, a0 = bc(1, s_), bc(2, s_), bc(3, s_), bc(4, s_), bc(5, s_)
        for x0, y0, n in ((XA0 + reg * SRA + a0, yreg + c0, a1 - a0),
                          (reg * SR + b0, yreg + c0 + (a1 - a0), b1 - b0)):
            adr = jnp.where(gidx >= gs, jnp.where(is_x, x0, y0) + 8.0 * (gidx - gs), adr)
            gs = gs + jnp.floor((n + 7.0) * 0.125)
    adr = jnp.where(gidx >= gs, jnp.where(is_x, float(XDUMP), float(YDUMP)), adr)
    ga_v[...] = adr.astype(jnp.int32)
    ga_cp = pltpu.make_async_copy(ga_v, ga_s, misc_sems.at[5])
    ga_cp.start()
    sc_v[...] = slot_c.astype(jnp.int32)
    sc_cp = pltpu.make_async_copy(sc_v, sc_s, misc_sems.at[4])
    sc_cp.start()

    def tab(qi, s, e):
        return tab_s[e, 4 * qi + s]

    def tot(qi, s, c):
        return tab(qi, s, c * E_LOC + E_LOC - 1)

    class Stream:
        def __init__(self, s, c):
            self.s, self.c = s, c
            self.n = tot(0, s, c)
            self.nc = _up(self.n, GC)
            self.nd = _up(tot(2, s, c), GD)
            self.na = _up(tot(6, s, c), GA)
            self.ud = (self.nd + PD - 1) // PD
            self.uc = (self.nc + PC - 1) // PC

        def _end(self, qi, j):
            return tab(qi, self.s, self.c * E_LOC + jnp.clip(j, 0, E_LOC - 1))

        def need(self, j):
            return jnp.where(j < 0, 0, jnp.minimum((self._end(2, j) + 7 + PD - 1) // PD, self.ud))

        def sched(self, j):
            u = jnp.maximum((self._end(2, j) + 7 + PD - 1) // PD, j + 1)
            return jnp.where(j < 0, 0, jnp.minimum(u, self.ud))

        def avail(self, j):
            a = jnp.where(j >= E_LOC - 1, self.uc, self._end(0, j) // PC)
            return jnp.where(j < 0, 0, a)

    sd_cp.wait()
    scatter_block(sd_s, NBA)
    tab_cp.wait()
    s_out = {k: Stream(me, me ^ k) for k in range(1, 4)}
    s_in = {k: Stream(me ^ k, me) for k in range(1, 4)}
    sx, sy = Stream(me ^ 3, me ^ 1), Stream(me ^ 1, me ^ 3)
    s_fd = {0: sx, 1: sy}
    s_fc = {0: sy, 1: sx}
    for sl in range(2):
        ap.forward(sl, s_fd[sl].na, 0, ap.sps)
    for i in range(NBA + 1, len(XBLK)):
        scatter_block(sd_s, i)
        if i == len(XBLK) - 2:
            for j in range(E_LOC):
                pltpu.make_async_copy(w_hbm.at[j], w_v.at[j], w_sems.at[j]).start(priority=1)

    def d_step(j):
        for sl in range(2):
            st = s_fd[sl]
            dp.forward(sl, st.nd, st.sched(j + LF - 1), st.sched(j + LF))
        for k, la in ((3, LD), (1, LD), (2, LH)):
            st = s_out[k]
            dp.send(k, st.nd, st.sched(j + la - 1), st.sched(j + la))

    def put_rows(k_region, k_tok, r0, r1):
        def grp8(g8, c):
            for u in range(8):
                r = jnp.minimum(r0 + g8 * 8 + u, r1 - 1)
                o = tok_s[k_tok * SR + r]
                w = ys[k_region * SR + r]
                out_v[o >> 3, 0:4, o & 7, :] = _lo(w)
                out_v[o >> 3, 4:8, o & 7, :] = _hi(w)
            return c
        lax.fori_loop(0, (r1 - r0 + 7) >> 3, grp8, 0)

    def recv_put(k, j):
        st = s_out[k]

        def fn(u, off, sz, ri):
            cp_.direct(k, u, off, sz, ri).wait_recv()
            put_rows(3 + k, k, off, jnp.minimum(off + sz, st.n))
        cp_.units(st.nc, st.avail(j - 1), st.avail(j), fn)

    def c_tail(j):
        for sl in range(2):
            st = s_fc[sl]
            cp_.forward(sl, st.nc, st.avail(j - FLAG - 1), st.avail(j - FLAG))
        for k in (3, 1):
            recv_put(k, j - PLAG)
        recv_put(2, j - PLAG - FLAG)

    z = jnp.int32(0)
    for k in (2, 3, 1):
        dp.send(k, s_out[k].nd, 0, s_out[k].sched(z))
    dp.send(2, s_out[2].nd, s_out[2].sched(z), s_out[2].sched(z + 1))

    f2 = 64 + (32 * (tot(2, 3, 0) - tot(2, 2, 1) + 2 * (tot(0, 0, 3) - tot(0, 1, 2)) + B1)
               ) // jnp.maximum(tot(0, 0, 2), 1)
    f0 = 64 - (32 * (tot(2, 3, 2) - tot(2, 0, 1) + 2 * (tot(0, 2, 3) - tot(0, 1, 0)) + B2)
               ) // jnp.maximum(tot(0, 2, 0), 1)
    cp_.frac = jnp.clip(f0, FLO, FHI) | (64 << 8) | (jnp.clip(f2, FLO, FHI) << 16) | (64 << 24)
    for k in (2, 3, 1):
        cnt_copy(me, k).wait_send()
    sc_cp.wait()
    ga_cp.wait()

    def zero(i, c):
        out_v[pl.ds(i * 4, 4)] = jnp.zeros((4, 8, 8, 128), f32)
        return c
    lax.fori_loop(0, N_TOK // 32, zero, 0)

    def pro(j, c):
        d_step(j)
        return c
    lax.fori_loop(-LF, 0, pro, 0)
    for k in (3, 1, 2):
        ap.wait(k, s_in[k].na, 0, ap.sps)

    def compute(j, c):
        e = me * E_LOC + j
        for k in (3, 1, 2):
            st = s_in[k]
            dp.wait(k, st.nd, st.need(j - 1), st.need(j))
        pltpu.make_async_copy(w_hbm.at[j], w_v.at[j], w_sems.at[j]).wait()
        xa = [ga_s[j, gi] for gi in range(NG)]
        ya = [ga_s[j, 32 + gi] for gi in range(NG)]
        w0 = jnp.concatenate([xs[pl.ds(a, 8), 0, :] for a in xa], axis=0)
        w1 = jnp.concatenate([xs[pl.ds(a, 8), 1, :] for a in xa], axis=0)
        lhs = jnp.concatenate([_lo(w0), _lo(w1), _hi(w0), _hi(w1)], axis=1).astype(bf16)
        for qq in range(4):
            wa = w_v[j, :, pl.ds(128 * qq, 128)].astype(bf16)
            wb = w_v[j, :, pl.ds(512 + 128 * qq, 128)].astype(bf16)
            pk = _pack(jnp.dot(lhs, wa, preferred_element_type=f32),
                       jnp.dot(lhs, wb, preferred_element_type=f32))
            for gi in range(NG):
                ys[pl.ds(ya[gi], 8), qq, :] = pk[8 * gi:8 * gi + 8]
        for k in (2, 3, 1):
            st = s_in[k]
            cp_.send(k, st.nc, st.avail(j - 1), st.avail(j))
        d_step(j)

        def tk(r, c2):
            for l in range(128):
                tok_s[sc_s[r, l]] = r * 128 + l
            return c2
        lax.fori_loop(jnp.clip(6 * (j - 1), 0, 16), jnp.clip(6 * j, 0, 16), tk, 0)

        @pl.when(j >= TOKS)
        def _():
            put_rows(0, 0, jnp.where(j == TOKS, 0, tab(1, me, e)), tab(0, me, e))
        c_tail(j)
        return c
    lax.fori_loop(0, E_LOC, compute, 0)

    ap.drain(a_out, {sl: s_fd[sl].na for sl in range(2)})
    dp.drain({k: s_out[k].nd for k in s_out}, {sl: s_fd[sl].nd for sl in range(2)})

    def ep(j, c):
        c_tail(j)
        return c
    lax.fori_loop(E_LOC, E_LOC + FLAG + PLAG - 1, ep, 0)
    cp_.drain({k: s_in[k].nc for k in s_in}, {sl: s_fc[sl].nc for sl in range(2)})
    recv_put(2, jnp.int32(E_LOC - 1))


def pallas_dist_moe_cap_ep_tokshard_n2048_d512_e8_h1024_kernel(
    x: jax.Array,
    router_W: jax.Array,
    route_idx: jax.Array,
    expert_W: jax.Array,
):
    del router_W
    idx = route_idx.astype(jnp.int32).reshape(16, 128)
    dma = pltpu.SemaphoreType.DMA
    i32 = jnp.int32
    out = pl.pallas_call(
        _body,
        out_shape=jax.ShapeDtypeStruct((N_TOK // 8, 8, 8, 128), f32),
        in_specs=[pl.BlockSpec(memory_space=pl.ANY)] * 3,
        out_specs=pl.BlockSpec(memory_space=pltpu.VMEM),
        scratch_shapes=[
            pltpu.VMEM((16, 128), i32),
            pltpu.VMEM((N_TOK, D), f32),
            pltpu.VMEM((E_LOC, D, H), f32),
            pltpu.VMEM((XDUMP + 8, 2, 128), u32),
            pltpu.VMEM((2 * (SR + SRA), 2, 128), u32),
            pltpu.VMEM((YDUMP + 8, 4, 128), u32),
            pltpu.VMEM((2 * SR, 4, 128), u32),
            pltpu.VMEM((8, 128), i32),
            pltpu.VMEM((16, 128), i32),
            pltpu.VMEM((16, 128), i32),
            pltpu.VMEM((8, 128), i32),
            pltpu.VMEM((N_DEV, E, 128), f32),
            pltpu.VMEM((E, 128), i32),
            pltpu.SMEM((8, 128), i32),
            pltpu.SMEM((16, 128), i32),
            pltpu.SMEM((16, 128), i32),
            pltpu.SMEM((8, 128), i32),
            pltpu.SMEM((E, 128), i32),
            pltpu.SMEM((YDUMP + 8,), i32),
            dma((6,)), dma((len(XBLK),)), dma((E_LOC,)), dma((3,)), dma((3,)),
            dma((3,)),
            dma((_n_sems(TA, PA, GA, 64),)),
            dma((_n_sems(MAXN, PD, GD, 64),)),
            dma((_n_sems(MAXN, PC, GC, max(FHI, 128 - FLO)),)),
        ],
        compiler_params=pltpu.CompilerParams(
            collective_id=0,
            vmem_limit_bytes=96 * 1024 * 1024,
            disable_semaphore_checks=True,
        ),
    )(x, idx, expert_W)
    return out.transpose(0, 2, 1, 3).reshape(N_TOK, H)
```

```python
import jax
import jax.numpy as jnp
from jax import lax
from jax.experimental import pallas as pl
from jax.experimental.pallas import tpu as pltpu

N_DEV = 4
N_TOK = 2048
D = 512
H = 1024
E_LOC = 8
E = 32
CAP = 204
NG = 32
MAXN = E_LOC * CAP
RA = 4
TA = RA * 128
MAXB = min(MAXN, N_TOK - TA)
PA, GA = 64, 8
PD, GD = 64, 8
PC, GC = 32, 4
SR = MAXN + 8
SRA = TA + 8
XA0 = 7 * SR
XDUMP = XA0 + 7 * SRA
YDUMP = 7 * SR
XBLK = ((0, 2), (2, 3), (3, 4), (4, 7), (7, 10), (10, 13), (13, 15), (15, 16))
NBA = 3
LF, LD, LH = 2, 3, 4
FLAG = 2
PLAG = 3
TOKS = 3
FLO, FHI = 40, 88
B1, B2 = 250, 150
MESH = pl.DeviceIdType.MESH
u32 = jnp.uint32
f32 = jnp.float32
bf16 = jnp.bfloat16


def _rem_sizes(p, g):
    out = []
    s = p // 2
    while s >= g:
        out.append(s)
        s //= 2
    return tuple(out)


def _sem_counts(maxn, p, g, fmax):
    nfull, nrem = maxn // p, len(_rem_sizes(p, g))
    return nfull + nrem, min(nfull, (nfull * fmax + 127) // 128 + 1) + nrem


def _n_sems(maxn, p, g, fmax):
    sps, fps = _sem_counts(maxn, p, g, fmax)
    return 3 * sps + 2 * fps


def _pack(a, b):
    ab = lax.bitcast_convert_type(a.astype(bf16).astype(f32), u32)
    bb = lax.bitcast_convert_type(b.astype(bf16).astype(f32), u32)
    return (ab >> 16) | bb


def _lo(w):
    return lax.bitcast_convert_type(w << 16, f32)


def _hi(w):
    return lax.bitcast_convert_type(w & jnp.uint32(0xFFFF0000), f32)


def _up(n, g):
    return (n + (g - 1)) & ~(g - 1)


def _body(x_hbm, idx_hbm, w_hbm, out_v,
          idx_v, x_v, w_v, xs, dfwd, ys, cfwd,
          sa_v, sd_v, sc_v, ga_v, cnt_v, tab_v, sa_s, sd_s, sc_s, ga_s, tab_s, tok_s,
          misc_sems, x_sems, w_sems, cnt_recv,
          send_sems, a_recv, d_recv, c_recv):
    me = lax.axis_index("i")

    idx_cp = pltpu.make_async_copy(idx_hbm, idx_v, misc_sems.at[0])
    idx_cp.start()
    x_cps = [pltpu.make_async_copy(x_hbm.at[pl.ds(128 * a, 128 * (b - a))],
                                   x_v.at[pl.ds(128 * a, 128 * (b - a))], x_sems.at[i])
             for i, (a, b) in enumerate(XBLK)]
    for cp in x_cps:
        cp.start(priority=1)
    bar = pltpu.get_barrier_semaphore()
    for k in range(1, N_DEV):
        pl.semaphore_signal(bar, inc=1, device_id=(me ^ k,), device_id_type=MESH)
    idx_cp.wait()

    idx = idx_v[...]
    onehot = [(idx == e) for e in range(E)]
    o_em = jnp.concatenate([jnp.where(o, 1.0, 0.0) for o in onehot], axis=0).astype(bf16)
    r_i = lax.broadcasted_iota(jnp.int32, (128, 256), 0)
    c_i = lax.broadcasted_iota(jnp.int32, (128, 256), 1)
    rhs1 = jnp.where(r_i < c_i, 1.0, 0.0).astype(bf16)
    g = jnp.dot(o_em, rhs1, preferred_element_type=f32)
    p_em = g[:, :128]
    t_em = g[:, 128:]
    t_l = jnp.concatenate([t_em[16 * e:16 * (e + 1)] for e in range(E)], axis=1).astype(bf16)
    r2 = lax.broadcasted_iota(jnp.int32, (32, 16), 0)
    c2 = lax.broadcasted_iota(jnp.int32, (32, 16), 1)
    lhs2 = jnp.where(c2 < jnp.where(r2 < 24, r2, RA), 1.0, 0.0).astype(bf16)
    h = jnp.dot(lhs2, t_l, preferred_element_type=f32)
    sub = lax.broadcasted_iota(jnp.int32, (8, 128), 0)
    rank = jnp.zeros((16, 128), f32)
    hist, hist_a = [], []
    for c in range(N_DEV):
        acc = jnp.zeros((8, 128), f32)
        acc_a = jnp.zeros((8, 128), f32)
        for j in range(E_LOC):
            e = c * E_LOC + j
            he = h[:, 128 * e:128 * (e + 1)]
            rank = jnp.where(onehot[e], p_em[16 * e:16 * (e + 1)] + he[:16], rank)
            acc = jnp.where(sub == j, he[16:24], acc)
            acc_a = jnp.where(sub == j, he[24:32], acc_a)
        hist.append(acc)
        hist_a.append(acc_a)
    cnt_me = jnp.minimum(jnp.concatenate(hist, axis=0), float(CAP))
    ca_me = jnp.minimum(jnp.concatenate(hist_a, axis=0), float(CAP))
    lane = lax.broadcasted_iota(jnp.int32, (E, 128), 1)
    row = lax.broadcasted_iota(jnp.int32, (E, 128), 0)
    cnt_v[me] = jnp.where(lane < 64, cnt_me, ca_me)

    r3 = lax.broadcasted_iota(jnp.int32, (E, E), 0)
    c3 = lax.broadcasted_iota(jnp.int32, (E, E), 1)
    tri = jnp.where((c3 < r3) & ((c3 >> 3) == (r3 >> 3)), 1.0, 0.0).astype(bf16)
    region = ((row >> 3) ^ me).astype(f32)
    ka_me = jnp.dot(tri, ca_me.astype(bf16), preferred_element_type=f32)
    base_a = ka_me + region * SRA + XA0
    end_a = ka_me + ca_me
    rank8 = rank[:8]
    slot_a = jnp.full((8, 128), float(XDUMP), f32)
    for e in range(E):
        slot_a = jnp.where(onehot[e][:8] & (rank8 < CAP),
                           rank8 + jnp.broadcast_to(base_a[e:e + 1], (8, 128)), slot_a)
    for c in range(N_DEV):
        e = c * E_LOC + E_LOC - 1
        slot_a = jnp.where(sub == 4 + c, jnp.broadcast_to(end_a[e:e + 1], (8, 128)), slot_a)
    sa_v[...] = slot_a.astype(jnp.int32)
    sa_cp = pltpu.make_async_copy(sa_v, sa_s, misc_sems.at[1])
    sa_cp.start()

    def cnt_copy(owner, k):
        return pltpu.make_async_remote_copy(
            src_ref=cnt_v.at[owner], dst_ref=cnt_v.at[owner],
            send_sem=send_sems.at[3], recv_sem=cnt_recv.at[k - 1],
            device_id=(me ^ k,), device_id_type=MESH)

    pl.semaphore_wait(bar, N_DEV - 1)
    for k in (2, 3, 1):
        cnt_copy(me, k).start()

    def scatter_block(slot_s, i):
        x_cps[i].wait()

        def sc(r, c):
            for g8 in range(16):
                xv = x_v[pl.ds(pl.multiple_of(r * 128 + 8 * g8, 8), 8), :]
                w0 = _pack(xv[:, 0:128], xv[:, 256:384])
                w1 = _pack(xv[:, 128:256], xv[:, 384:512])
                for u in range(8):
                    sl = slot_s[r, 8 * g8 + u]
                    xs[sl, 0:1, :] = w0[u:u + 1]
                    xs[sl, 1:2, :] = w1[u:u + 1]
            return c
        lax.fori_loop(XBLK[i][0], XBLK[i][1], sc, 0)

    class Phase:
        def __init__(self, buf, base, reg, fwd, fbase, recv, ssem, p, g, maxn, fmax):
            self.buf, self.base, self.reg, self.fwd, self.fbase = buf, base, reg, fwd, fbase
            self.recv, self.ssem, self.p, self.g = recv, ssem, p, g
            self.sps, self.fps = _sem_counts(maxn, p, g, fmax)
            self.nrem = len(_rem_sizes(p, g))
            self.frac = jnp.int32(0x40404040)

        def units(self, n, u0, u1, fn):
            nf = n // self.p

            def body(u, c):
                fn(u, u * self.p, self.p, None)
                return c
            lax.fori_loop(u0, jnp.minimum(u1, nf), body, 0)
            rem = n - nf * self.p

            @pl.when((u0 <= nf) & (nf < u1))
            def _():
                for i, sz in enumerate(_rem_sizes(self.p, self.g)):
                    @pl.when((rem & sz) != 0)
                    def _(i=i, sz=sz):
                        fn(nf, nf * self.p + (rem & ~(2 * sz - 1)), sz, i)

        def n_x(self, a, u):
            return (u * ((self.frac >> (8 * a)) & 255) + 32) >> 7

        def via_x(self, a, u):
            return self.n_x(a, u + 1) - self.n_x(a, u)

        def rows(self, region_, off, sz):
            return self.buf.at[pl.ds(self.base + region_ * self.reg + off, sz)]

        def frows(self, sl, off, sz):
            return self.fwd.at[pl.ds(self.fbase + sl * self.reg + off, sz)]

        def sem(self, k, u, ri):
            return self.recv.at[(k - 1) * self.sps + (u if ri is None else self.sps - self.nrem + ri)]

        def direct(self, k, u, off, sz, ri):
            return pltpu.make_async_remote_copy(
                src_ref=self.rows(k, off, sz), dst_ref=self.rows(3 + k, off, sz),
                send_sem=send_sems.at[self.ssem], recv_sem=self.sem(k, u, ri),
                device_id=(me ^ k,), device_id_type=MESH)

        def hop1(self, a, sl, u, off, sz, ri):
            if ri is None:
                nx = self.n_x(a, u)
                si = jnp.where(sl == 0, nx, u - nx)
            else:
                si = self.fps - self.nrem + ri
            return pltpu.make_async_remote_copy(
                src_ref=self.rows(2, off, sz), dst_ref=self.frows(sl, off, sz),
                send_sem=send_sems.at[self.ssem],
                recv_sem=self.recv.at[3 * self.sps + sl * self.fps + si],
                device_id=(me ^ (3 - 2 * sl),), device_id_type=MESH)

        def hop1_out(self, u, off, sz, ri):
            return self.hop1(me, 1 - self.via_x(me, u), u, off, sz, ri)

        def hop2(self, sl, u, off, sz, ri):
            return pltpu.make_async_remote_copy(
                src_ref=self.frows(sl, off, sz), dst_ref=self.rows(5, off, sz),
                send_sem=send_sems.at[self.ssem], recv_sem=self.sem(2, u, ri),
                device_id=(me ^ (1 + 2 * sl),), device_id_type=MESH)

        def mine(self, sl, u):
            return self.via_x(me ^ (3 - 2 * sl), u) == 1 - sl

        def send(self, k, n, u0, u1):
            if k == 2:
                self.units(n, u0, u1, lambda *a: self.hop1_out(*a).start())
            else:
                self.units(n, u0, u1, lambda *a: self.direct(k, *a).start())

        def wait(self, k, n, u0, u1):
            self.units(n, u0, u1, lambda *a: self.direct(k, *a).wait_recv())

        def forward(self, sl, n, u0, u1):
            def fn(u, off, sz, ri):
                @pl.when(self.mine(sl, u))
                def _():
                    self.hop1(me ^ (3 - 2 * sl), sl, u, off, sz, ri).wait_recv()
                    self.hop2(sl, u, off, sz, ri).start()
            self.units(n, u0, u1, fn)

        def drain(self, own, fwd):
            self.units(own[2], 0, self.sps, lambda *a: self.hop1_out(*a).wait_send())
            for k in (3, 1):
                self.units(own[k], 0, self.sps, lambda *a, k=k: self.direct(k, *a).wait_send())
            for sl in range(2):
                def fn(u, off, sz, ri, sl=sl):
                    @pl.when(self.mine(sl, u))
                    def _():
                        self.hop2(sl, u, off, sz, ri).wait_send()
                self.units(fwd[sl], 0, self.sps, fn)

    ap = Phase(xs, XA0, SRA, dfwd, 2 * SR, a_recv, 0, PA, GA, TA, 64)
    dp = Phase(xs, 0, SR, dfwd, 0, d_recv, 1, PD, GD, MAXB, 64)
    cp_ = Phase(ys, 0, SR, cfwd, 0, c_recv, 2, PC, GC, MAXN, max(FHI, 128 - FLO))

    sa_cp.wait()
    for i in range(NBA):
        scatter_block(sa_s, i)
    a_out = {k: _up(sa_s[4 + (me ^ k), 0], GA) for k in range(1, 4)}
    for k in (2, 3, 1):
        ap.send(k, a_out[k], 0, ap.sps)

    for k in range(1, N_DEV):
        cnt_copy(me ^ k, k).wait_recv()
    pre = jnp.zeros((E, 128), f32)
    q = jnp.zeros((E, 128), f32)
    add = jnp.zeros((E, 128), f32)
    nk_me = jnp.zeros((E, 128), f32)
    grp = lane >> 2
    for s in range(N_DEV):
        m = cnt_v[s]
        mr = pltpu.roll(m, 64, 1)
        c = jnp.where(lane < 64, m, mr)
        ca = jnp.where(lane < 64, mr, m)
        nk = jnp.clip(CAP - pre, 0.0, c)
        pre = pre + c
        na = jnp.minimum(ca, nk)
        nb = nk - na
        sel = (lane & 3) == s
        qs = jnp.where(grp < 2, nk, jnp.where(grp < 4, nb, ca))
        ads = jnp.where(grp == 0, nk, jnp.where(grp == 2, nb,
                        jnp.where(grp == 4, na, jnp.where(grp == 6, ca, 0.0))))
        q = jnp.where(sel, qs, q)
        add = jnp.where(sel, ads, add)
        nk_me = jnp.where(me == s, nk, nk_me)
    nb_me = nk_me - jnp.minimum(ca_me, nk_me)
    kk = jnp.dot(tri, jnp.concatenate([nb_me, q, nk_me], axis=1).astype(bf16),
                 preferred_element_type=f32)
    base_d = kk[:, :128] + region * SR - ca_me
    base_c = kk[:, 256:] + region * SR
    slot_d = jnp.full((16, 128), float(XDUMP), f32)
    slot_c = jnp.full((16, 128), float(YDUMP), f32)
    for e in range(E):
        keep = onehot[e] & (rank < jnp.broadcast_to(nk_me[e:e + 1], (16, 128)))
        slot_d = jnp.where(keep, rank + jnp.broadcast_to(base_d[e:e + 1], (16, 128)), slot_d)
        slot_c = jnp.where(keep, rank + jnp.broadcast_to(base_c[e:e + 1], (16, 128)), slot_c)
    sd_v[...] = slot_d.astype(jnp.int32)
    sd_cp = pltpu.make_async_copy(sd_v, sd_s, misc_sems.at[0])
    sd_cp.start()
    tabf = kk[:, 128:256] + add
    tab_v[...] = tabf.astype(jnp.int32)
    tab_cp = pltpu.make_async_copy(tab_v, tab_s, misc_sems.at[1])
    tab_cp.start()

    t = tabf[:8]
    for c in range(1, N_DEV):
        t = jnp.where(me == c, tabf[8 * c:8 * c + 8], t)
    lane8 = lax.broadcasted_iota(jnp.int32, (8, 128), 1)
    is_x = lane8 < 32
    gidx = (lane8 & 31).astype(f32)

    def bc(qi, s_):
        return jnp.broadcast_to(t[:, 4 * qi + s_:4 * qi + s_ + 1], (8, 128))
    gs = jnp.zeros((8, 128), f32)
    adr = jnp.zeros((8, 128), f32)
    for s_ in range(N_DEV):
        kx = s_ ^ me
        reg = jnp.where(kx == 0, 0, 3 + kx).astype(f32)
        yreg = (kx * SR).astype(f32)
        c0, b1, b0, a1, a0 = bc(1, s_), bc(2, s_), bc(3, s_), bc(4, s_), bc(5, s_)
        for x0, y0, n in ((XA0 + reg * SRA + a0, yreg + c0, a1 - a0),
                          (reg * SR + b0, yreg + c0 + (a1 - a0), b1 - b0)):
            adr = jnp.where(gidx >= gs, jnp.where(is_x, x0, y0) + 8.0 * (gidx - gs), adr)
            gs = gs + jnp.floor((n + 7.0) * 0.125)
    adr = jnp.where(gidx >= gs, jnp.where(is_x, float(XDUMP), float(YDUMP)), adr)
    ga_v[...] = adr.astype(jnp.int32)
    ga_cp = pltpu.make_async_copy(ga_v, ga_s, misc_sems.at[2])
    ga_cp.start()
    sc_v[...] = slot_c.astype(jnp.int32)
    sc_cp = pltpu.make_async_copy(sc_v, sc_s, misc_sems.at[3])
    sc_cp.start()

    def tab(qi, s, e):
        return tab_s[e, 4 * qi + s]

    def tot(qi, s, c):
        return tab(qi, s, c * E_LOC + E_LOC - 1)

    class Stream:
        def __init__(self, s, c):
            self.s, self.c = s, c
            self.n = tot(0, s, c)
            self.nc = _up(self.n, GC)
            self.nd = _up(tot(2, s, c), GD)
            self.na = _up(tot(6, s, c), GA)
            self.ud = (self.nd + PD - 1) // PD
            self.uc = (self.nc + PC - 1) // PC

        def _end(self, qi, j):
            return tab(qi, self.s, self.c * E_LOC + jnp.clip(j, 0, E_LOC - 1))

        def need(self, j):
            return jnp.where(j < 0, 0, jnp.minimum((self._end(2, j) + 7 + PD - 1) // PD, self.ud))

        def sched(self, j):
            u = jnp.maximum((self._end(2, j) + 7 + PD - 1) // PD, j + 1)
            return jnp.where(j < 0, 0, jnp.minimum(u, self.ud))

        def avail(self, j):
            a = jnp.where(j >= E_LOC - 1, self.uc, self._end(0, j) // PC)
            return jnp.where(j < 0, 0, a)

    sd_cp.wait()
    scatter_block(sd_s, NBA)
    tab_cp.wait()
    s_out = {k: Stream(me, me ^ k) for k in range(1, 4)}
    s_in = {k: Stream(me ^ k, me) for k in range(1, 4)}
    sx, sy = Stream(me ^ 3, me ^ 1), Stream(me ^ 1, me ^ 3)
    s_fd = {0: sx, 1: sy}
    s_fc = {0: sy, 1: sx}
    for sl in range(2):
        ap.forward(sl, s_fd[sl].na, 0, ap.sps)
    for i in range(NBA + 1, len(XBLK)):
        scatter_block(sd_s, i)
        if i == len(XBLK) - 2:
            for j in range(E_LOC):
                pltpu.make_async_copy(w_hbm.at[j], w_v.at[j], w_sems.at[j]).start(priority=1)

    def d_step(j):
        for sl in range(2):
            st = s_fd[sl]
            dp.forward(sl, st.nd, st.sched(j + LF - 1), st.sched(j + LF))
        for k, la in ((3, LD), (1, LD), (2, LH)):
            st = s_out[k]
            dp.send(k, st.nd, st.sched(j + la - 1), st.sched(j + la))

    def put_rows(k_region, k_tok, r0, r1):
        def grp8(g8, c):
            for u in range(8):
                r = jnp.minimum(r0 + g8 * 8 + u, r1 - 1)
                o = tok_s[k_tok * SR + r]
                w = ys[k_region * SR + r]
                out_v[o >> 3, 0:4, o & 7, :] = _lo(w)
                out_v[o >> 3, 4:8, o & 7, :] = _hi(w)
            return c
        lax.fori_loop(0, (r1 - r0 + 7) >> 3, grp8, 0)

    def recv_put(k, j):
        st = s_out[k]

        def fn(u, off, sz, ri):
            cp_.direct(k, u, off, sz, ri).wait_recv()
            put_rows(3 + k, k, off, jnp.minimum(off + sz, st.n))
        cp_.units(st.nc, st.avail(j - 1), st.avail(j), fn)

    def c_tail(j):
        for sl in range(2):
            st = s_fc[sl]
            cp_.forward(sl, st.nc, st.avail(j - FLAG - 1), st.avail(j - FLAG))
        for k in (3, 1):
            recv_put(k, j - PLAG)
        recv_put(2, j - PLAG - FLAG)

    z = jnp.int32(0)
    for k in (2, 3, 1):
        dp.send(k, s_out[k].nd, 0, s_out[k].sched(z))
    dp.send(2, s_out[2].nd, s_out[2].sched(z), s_out[2].sched(z + 1))

    f2 = 64 + (32 * (tot(2, 3, 0) - tot(2, 2, 1) + 2 * (tot(0, 0, 3) - tot(0, 1, 2)) + B1)
               ) // jnp.maximum(tot(0, 0, 2), 1)
    f0 = 64 - (32 * (tot(2, 3, 2) - tot(2, 0, 1) + 2 * (tot(0, 2, 3) - tot(0, 1, 0)) + B2)
               ) // jnp.maximum(tot(0, 2, 0), 1)
    cp_.frac = jnp.clip(f0, FLO, FHI) | (64 << 8) | (jnp.clip(f2, FLO, FHI) << 16) | (64 << 24)
    for k in (2, 3, 1):
        cnt_copy(me, k).wait_send()
    sc_cp.wait()
    ga_cp.wait()

    def zero(i, c):
        out_v[pl.ds(i * 4, 4)] = jnp.zeros((4, 8, 8, 128), f32)
        return c
    lax.fori_loop(0, N_TOK // 32, zero, 0)

    def pro(j, c):
        d_step(j)
        return c
    lax.fori_loop(-LF, 0, pro, 0)
    for k in (3, 1, 2):
        ap.wait(k, s_in[k].na, 0, ap.sps)

    def compute(j, c):
        e = me * E_LOC + j
        for k in (3, 1, 2):
            st = s_in[k]
            dp.wait(k, st.nd, st.need(j - 1), st.need(j))
        pltpu.make_async_copy(w_hbm.at[j], w_v.at[j], w_sems.at[j]).wait()
        xa = [ga_s[j, gi] for gi in range(NG)]
        ya = [ga_s[j, 32 + gi] for gi in range(NG)]
        w0 = jnp.concatenate([xs[pl.ds(a, 8), 0, :] for a in xa], axis=0)
        w1 = jnp.concatenate([xs[pl.ds(a, 8), 1, :] for a in xa], axis=0)
        lhs = jnp.concatenate([_lo(w0), _lo(w1), _hi(w0), _hi(w1)], axis=1).astype(bf16)
        for qq in range(4):
            wa = w_v[j, :, pl.ds(128 * qq, 128)].astype(bf16)
            wb = w_v[j, :, pl.ds(512 + 128 * qq, 128)].astype(bf16)
            pk = _pack(jnp.dot(lhs, wa, preferred_element_type=f32),
                       jnp.dot(lhs, wb, preferred_element_type=f32))
            for gi in range(NG):
                ys[pl.ds(ya[gi], 8), qq, :] = pk[8 * gi:8 * gi + 8]
        for k in (2, 3, 1):
            st = s_in[k]
            cp_.send(k, st.nc, st.avail(j - 1), st.avail(j))
        d_step(j)

        def tk(r, c2):
            for l in range(128):
                tok_s[sc_s[r, l]] = r * 128 + l
            return c2
        lax.fori_loop(jnp.clip(6 * (j - 1), 0, 16), jnp.clip(6 * j, 0, 16), tk, 0)

        @pl.when(j >= TOKS)
        def _():
            put_rows(0, 0, jnp.where(j == TOKS, 0, tab(1, me, e)), tab(0, me, e))
        c_tail(j)
        return c
    lax.fori_loop(0, E_LOC, compute, 0)

    ap.drain(a_out, {sl: s_fd[sl].na for sl in range(2)})
    dp.drain({k: s_out[k].nd for k in s_out}, {sl: s_fd[sl].nd for sl in range(2)})

    def ep(j, c):
        c_tail(j)
        return c
    lax.fori_loop(E_LOC, E_LOC + FLAG + PLAG - 1, ep, 0)
    cp_.drain({k: s_in[k].nc for k in s_in}, {sl: s_fc[sl].nc for sl in range(2)})
    recv_put(2, jnp.int32(E_LOC - 1))


def pallas_dist_moe_cap_ep_tokshard_n2048_d512_e8_h1024_kernel(
    x: jax.Array,
    router_W: jax.Array,
    route_idx: jax.Array,
    expert_W: jax.Array,
):
    del router_W
    idx = route_idx.astype(jnp.int32).reshape(16, 128)
    dma = pltpu.SemaphoreType.DMA
    i32 = jnp.int32
    out = pl.pallas_call(
        _body,
        out_shape=jax.ShapeDtypeStruct((N_TOK // 8, 8, 8, 128), f32),
        in_specs=[pl.BlockSpec(memory_space=pl.ANY)] * 3,
        out_specs=pl.BlockSpec(memory_space=pltpu.VMEM),
        scratch_shapes=[
            pltpu.VMEM((16, 128), i32),
            pltpu.VMEM((N_TOK, D), f32),
            pltpu.VMEM((E_LOC, D, H), f32),
            pltpu.VMEM((XDUMP + 8, 2, 128), u32),
            pltpu.VMEM((2 * (SR + SRA), 2, 128), u32),
            pltpu.VMEM((YDUMP + 8, 4, 128), u32),
            pltpu.VMEM((2 * SR, 4, 128), u32),
            pltpu.VMEM((8, 128), i32),
            pltpu.VMEM((16, 128), i32),
            pltpu.VMEM((16, 128), i32),
            pltpu.VMEM((8, 128), i32),
            pltpu.VMEM((N_DEV, E, 128), f32),
            pltpu.VMEM((E, 128), i32),
            pltpu.SMEM((8, 128), i32),
            pltpu.SMEM((16, 128), i32),
            pltpu.SMEM((16, 128), i32),
            pltpu.SMEM((8, 128), i32),
            pltpu.SMEM((E, 128), i32),
            pltpu.SMEM((YDUMP + 8,), i32),
            dma((4,)), dma((len(XBLK),)), dma((E_LOC,)), dma((3,)),
            dma((4,)),
            dma((_n_sems(TA, PA, GA, 64),)),
            dma((_n_sems(MAXB, PD, GD, 64),)),
            dma((_n_sems(MAXN, PC, GC, max(FHI, 128 - FLO)),)),
        ],
        compiler_params=pltpu.CompilerParams(
            collective_id=0,
            vmem_limit_bytes=96 * 1024 * 1024,
            disable_semaphore_checks=True,
        ),
    )(x, idx, expert_W)
    return out.transpose(0, 2, 1, 3).reshape(N_TOK, H)
```
